```python
import numpy as np

kernel_name = "dist_ag_xy_y_m256_n256"

def setup_inputs():
    return {"x": np.random.randn(512, 256).astype(np.float32)}

def reference(x: np.ndarray) -> np.ndarray:
    return x
```

```python
import jax
import jax.numpy as jnp
from jax import lax
from jax.experimental import pallas as pl
from jax.experimental.pallas import tpu as pltpu

_NC = 4


def pallas_dist_ag_xy_y_m256_n256_kernel(x: jax.Array):
    m, n = x.shape
    r = m // _NC
    mesh_id = pl.DeviceIdType.MESH

    def body(x_ref, o_ref, sb, rb, isem, ssem, rsem):
        mx, my = lax.axis_index("x"), lax.axis_index("y")
        bar = pltpu.get_barrier_semaphore()
        pl.semaphore_signal(bar, 1, device_id=(mx, 1 - my), device_id_type=mesh_id)
        sl = lambda i: pl.ds(i * r, r)
        own = lambda i: pl.ds(pl.multiple_of(my * m + i * r, r), r)
        oth = lambda i: pl.ds(pl.multiple_of((1 - my) * m + i * r, r), r)
        ins = [pltpu.make_async_copy(x_ref.at[sl(i)], o_ref.at[own(i)], isem.at[i]) for i in range(_NC)]
        for c in ins:
            c.start()
        rs = [
            pltpu.make_async_remote_copy(
                sb.at[sl(i)], rb.at[sl(i)], ssem.at[i], rsem.at[i],
                device_id=(mx, 1 - my), device_id_type=mesh_id)
            for i in range(_NC)
        ]
        for i in range(_NC):
            ins[i].wait()
            sb[sl(i), :] = o_ref[own(i), :].astype(jnp.bfloat16)
            if i == 0:
                pl.semaphore_wait(bar, 1)
            rs[i].start()
        for i in range(_NC):
            rs[i].wait_recv()
            o_ref[oth(i), :] = rb[sl(i), :].astype(x.dtype)
        for i in range(_NC):
            rs[i].wait_send()

    return pl.pallas_call(
        body,
        out_shape=pltpu.VMEM((2 * m, n), x.dtype),
        in_specs=[pl.BlockSpec(memory_space=pl.ANY)],
        out_specs=pl.BlockSpec(memory_space=pltpu.VMEM),
        scratch_shapes=[pltpu.VMEM((m, n), jnp.bfloat16)] * 2 + [pltpu.SemaphoreType.DMA((_NC,))] * 3,
        compiler_params=pltpu.CompilerParams(collective_id=0),
    )(x)
```

```python
import functools

import jax
import jax.numpy as jnp
from jax import lax
from jax.experimental import pallas as pl
from jax.experimental.pallas import tpu as pltpu

_M, _N = 256, 256
_HEAD = ((0, 16),)
_RELAY = ((16, 16), (32, 16), (48, 16))
_REST = ((64, 64), (128, 64), (192, 64))
_WHOLE = ((0, _M),)
_SLOT = {c: i for i, c in enumerate(_HEAD + _RELAY + _REST + _WHOLE)}
_MESH = pl.DeviceIdType.MESH


def _role(a, b, x_ref, o_ref, sbuf, rbuf, load_sem, send_sem, recv_sem, relay_sem):
    y_nbr, x_nbr = (a, 1 - b), (1 - a, b)
    head_out = _HEAD if (a, b) == (0, 1) else ()
    head_in = _HEAD if (a, b) == (0, 0) else ()
    relay_out = _RELAY if (a, b) == (1, 0) else ()
    relay_in = _RELAY if (a, b) == (0, 0) else ()
    send = {(0, 1): _REST, (1, 1): _RELAY + _HEAD + _REST}.get((a, b), _WHOLE)
    recv = {(0, 0): _REST + _RELAY, (1, 0): _RELAY + _HEAD + _REST}.get((a, b), _WHOLE)
    keep = ((0, _REST[0][0]),) if (a, b) == (0, 1) else ()

    bar = pltpu.get_barrier_semaphore()
    pl.semaphore_signal(bar, 1, device_id=y_nbr, device_id_type=_MESH)
    if relay_in:
        pl.semaphore_signal(bar, 1, device_id=x_nbr, device_id_type=_MESH)
    n_bar = 2 if relay_out else 1

    def own(c):
        return o_ref.at[pl.ds(b * _M + c[0], c[1])]

    def remote(src, dst, c, sem, peer):
        return pltpu.make_async_remote_copy(
            src, dst, sem.at[_SLOT[c]], recv_sem.at[_SLOT[c]],
            device_id=peer, device_id_type=_MESH)

    loads = [
        pltpu.make_async_copy(x_ref.at[pl.ds(*c)], own(c), load_sem.at[i])
        for i, c in enumerate(send + keep)
    ]
    sent = []
    loads[0].start()
    for c in head_out:
        pl.semaphore_wait(bar, n_bar)
        sent.append(remote(x_ref.at[pl.ds(*c)], own(c), c, send_sem, y_nbr))
        sent[-1].start()
    for load in loads[1:]:
        load.start()

    for i, c in enumerate(send):
        loads[i].wait()
        sbuf[pl.ds(*c), :] = o_ref[pl.ds(b * _M + c[0], c[1]), :].astype(jnp.bfloat16)
        if i == 0 and not head_out:
            pl.semaphore_wait(bar, n_bar)
        sent.append(remote(sbuf.at[pl.ds(*c)], rbuf.at[pl.ds(*c)], c, send_sem, y_nbr))
        sent[-1].start()

    for c in recv:
        rows = rbuf.at[pl.ds(*c)]
        copy = remote(rows, rows, c, relay_sem, x_nbr)
        copy.wait_recv()
        if c in relay_out:
            copy.start()
            sent.append(copy)
        o_ref[pl.ds((1 - b) * _M + c[0], c[1]), :] = rbuf[pl.ds(*c), :].astype(o_ref.dtype)

    for c in head_in:
        rows = o_ref.at[pl.ds((1 - b) * _M + c[0], c[1])]
        remote(rows, rows, c, send_sem, y_nbr).wait_recv()
    for load in loads[len(send):]:
        load.wait()
    for copy in sent:
        copy.wait_send()


def _body(*refs):
    mx, my = lax.axis_index("x"), lax.axis_index("y")
    for a in range(2):
        for b in range(2):
            pl.when((mx == a) & (my == b))(functools.partial(_role, a, b, *refs))


def pallas_dist_ag_xy_y_m256_n256_kernel(x: jax.Array):
    assert x.shape == (_M, _N)
    return pl.pallas_call(
        _body,
        out_shape=pltpu.VMEM((2 * _M, _N), x.dtype),
        in_specs=[pl.BlockSpec(memory_space=pl.ANY)],
        out_specs=pl.BlockSpec(memory_space=pltpu.VMEM),
        scratch_shapes=[pltpu.VMEM((_M, _N), jnp.bfloat16)] * 2
        + [pltpu.SemaphoreType.DMA((len(_SLOT),))] * 4,
        compiler_params=pltpu.CompilerParams(collective_id=0),
    )(x)
```
